```python
import numpy as np

kernel_name = "dist_sum_ax0_xy_m2048_n1024"

def setup_inputs():
    return {"x": np.random.randn(4096, 2048).astype(np.float32)}

def reference(x: np.ndarray) -> np.ndarray:
    return np.sum(x, axis=0, keepdims=True)
```

```python
import jax
import jax.numpy as jnp
from jax import lax
from jax.experimental import pallas as pl
from jax.experimental.pallas import tpu as pltpu

SUBLANES, LANES = 8, 128
MESH = pl.DeviceIdType.MESH

RAW_ROWS = 88
SMALL_CHUNKS = (256, 128, 64)
TAIL_ROWS = 64
UNROLL_ROWS = 64


def _tree_sum(values):
    values = list(values)
    while len(values) > 1:
        pairs = [values[i] + values[i + 1] for i in range(0, len(values) - 1, 2)]
        values = pairs + values[2 * len(pairs):]
    return values[0]


def _add_rows(ref, row0, rows, accs):
    accs = list(accs)
    for r in range(0, rows, SUBLANES):
        for j in range(len(accs)):
            accs[j] = accs[j] + ref[pl.ds(row0 + r, SUBLANES), pl.ds(j * LANES, LANES)]
    return accs


def _accumulate(ref, row0, rows, accs):
    trips = rows // UNROLL_ROWS
    if trips < 2:
        return _add_rows(ref, row0, rows, accs)

    def step(i, accs):
        base = pl.multiple_of(row0 + i * UNROLL_ROWS, SUBLANES)
        return tuple(_add_rows(ref, base, UNROLL_ROWS, accs))

    accs = lax.fori_loop(0, trips, step, tuple(accs))
    done = trips * UNROLL_ROWS
    return _add_rows(ref, row0 + done, rows - done, accs)


def pallas_dist_sum_ax0_xy_m2048_n1024_kernel(
    x: jax.Array,
):
    m, n = x.shape
    tiles = n // LANES
    local_rows = m - RAW_ROWS
    chunks = (local_rows - sum(SMALL_CHUNKS) - TAIL_ROWS, *SMALL_CHUNKS)
    starts = [sum(chunks[:i]) for i in range(len(chunks))]
    tail0 = local_rows - TAIL_ROWS

    def body(x_ref, o_ref, buf, raw, send, recv, chunk_sems, tail_sems,
             send_sem, recv_sem, raw_send_sem, raw_recv_sem):
        peer = (1 - lax.axis_index("x"), lax.axis_index("y"))
        cols = [pl.ds(j * LANES, LANES) for j in range(tiles)]
        tail = pl.ds(tail0, TAIL_ROWS)

        chunk_loads = [
            pltpu.make_async_copy(
                x_ref.at[pl.ds(r0, rows)], buf.at[pl.ds(r0, rows)], chunk_sems.at[i]
            )
            for i, (r0, rows) in enumerate(zip(starts, chunks))
        ]
        tail_loads = [
            pltpu.make_async_copy(
                x_ref.at[tail, cols[j]], buf.at[tail, cols[j]], tail_sems.at[j]
            )
            for j in range(tiles)
        ]
        for load in chunk_loads + tail_loads:
            load.start()

        barrier = pltpu.get_barrier_semaphore()
        pl.semaphore_signal(barrier, inc=1, device_id=peer, device_id_type=MESH)
        pl.semaphore_wait(barrier, 1)

        raw_copy = pltpu.make_async_remote_copy(
            x_ref.at[pl.ds(local_rows, RAW_ROWS)], raw, raw_send_sem, raw_recv_sem,
            device_id=peer, device_id_type=MESH,
        )
        raw_copy.start()

        accs = [jnp.zeros((SUBLANES, LANES), jnp.float32)] * tiles
        for i, load in enumerate(chunk_loads):
            load.wait()
            accs = _accumulate(buf, starts[i], chunks[i], accs)
            if i == 2:
                raw_copy.wait()
                accs = _accumulate(raw, 0, RAW_ROWS, accs)

        for j, load in enumerate(tail_loads):
            load.wait()
            acc = accs[j] + _tree_sum(
                buf[pl.ds(tail0 + r, SUBLANES), cols[j]]
                for r in range(0, TAIL_ROWS, SUBLANES)
            )
            send[:, cols[j]] = jnp.sum(acc, axis=0, keepdims=True)
            pltpu.make_async_remote_copy(
                send.at[:, cols[j]], recv.at[:, cols[j]], send_sem, recv_sem,
                device_id=peer, device_id_type=MESH,
            ).start()

        pltpu.make_async_copy(send, send, send_sem).wait()
        pltpu.make_async_copy(recv, recv, recv_sem).wait()
        o_ref[...] = send[...] + recv[...]

    return pl.pallas_call(
        body,
        out_shape=jax.ShapeDtypeStruct((1, n), jnp.float32),
        in_specs=[pl.BlockSpec(memory_space=pl.ANY)],
        out_specs=pl.BlockSpec(memory_space=pltpu.VMEM),
        scratch_shapes=[
            pltpu.VMEM((local_rows, n), jnp.float32),
            pltpu.VMEM((RAW_ROWS, n), jnp.float32),
            pltpu.VMEM((1, n), jnp.float32),
            pltpu.VMEM((1, n), jnp.float32),
            pltpu.SemaphoreType.DMA((len(chunks),)),
            pltpu.SemaphoreType.DMA((tiles,)),
            pltpu.SemaphoreType.DMA,
            pltpu.SemaphoreType.DMA,
            pltpu.SemaphoreType.DMA,
            pltpu.SemaphoreType.DMA,
        ],
        compiler_params=pltpu.CompilerParams(
            collective_id=0,
            disable_bounds_checks=True,
            disable_semaphore_checks=True,
        ),
    )(x)
```

```python
import jax
import jax.numpy as jnp
from jax import lax
from jax.experimental import pallas as pl
from jax.experimental.pallas import tpu as pltpu

SUBLANES, LANES = 8, 128
MESH = pl.DeviceIdType.MESH

STREAMS = 7
RAW_ROWS = 120
LAST_BATCHES = (4, 1)
STEPS_BEFORE_HANDSHAKE = 10


def _tree_sum(values):
    while len(values) > 1:
        pairs = [values[i] + values[i + 1] for i in range(0, len(values) - 1, 2)]
        values = pairs + values[2 * len(pairs):]
    return values[0]


def pallas_dist_sum_ax0_xy_m2048_n1024_kernel(
    x: jax.Array,
):
    m, n = x.shape
    block_rows = m // (STREAMS + 1)
    head_rows = block_rows - RAW_ROWS
    last_step = block_rows // SUBLANES - 1
    batches = (last_step - sum(LAST_BATCHES), *LAST_BATCHES)
    batch_of_step = [b for b, steps in enumerate(batches) for _ in range(steps)]
    tiles = n // LANES
    tail = [(0, STREAMS, t) for t in range(tiles - 1)]
    tail += [(0, STREAMS - 1, tiles - 1), (STREAMS - 1, 1, tiles - 1)]

    def body(x_ref, o_ref, steps_buf, head_buf, peer_rows, own_rows, send_buf, recv_buf,
             batch_sems, tail_sems, head_sem, own_sem, raw_send_sem, raw_recv_sem,
             send_sem, recv_sem):
        peer = (1 - lax.axis_index("x"), lax.axis_index("y"))
        cols = [pl.ds(t * LANES, LANES) for t in range(tiles)]
        raw_rows = x_ref.at[STREAMS, pl.ds(head_rows, RAW_ROWS)]

        def start_step(s):
            pltpu.make_async_copy(
                x_ref.at[pl.ds(0, STREAMS), pl.ds(s * SUBLANES, SUBLANES)],
                steps_buf.at[s],
                batch_sems.at[batch_of_step[s]],
            ).start()

        def wait_all(buf, sem):
            pltpu.make_async_copy(buf, buf, sem).wait()

        def add_step(s, accs):
            for i in range(STREAMS):
                accs = tuple(a + steps_buf[s, i, :, c] for a, c in zip(accs, cols))
            return accs

        def add_rows(buf, accs):
            for r in range(0, buf.shape[0], SUBLANES):
                accs = tuple(a + buf[pl.ds(r, SUBLANES), c] for a, c in zip(accs, cols))
            return accs

        head_load = pltpu.make_async_copy(
            x_ref.at[STREAMS, pl.ds(0, head_rows)], head_buf, head_sem
        )
        own_load = pltpu.make_async_copy(raw_rows, own_rows, own_sem)
        raw_copy = pltpu.make_async_remote_copy(
            raw_rows, peer_rows, raw_send_sem, raw_recv_sem,
            device_id=peer, device_id_type=MESH,
        )
        tail_loads = [
            pltpu.make_async_copy(
                x_ref.at[pl.ds(i, k), pl.ds(last_step * SUBLANES, SUBLANES), cols[t]],
                steps_buf.at[last_step, pl.ds(i, k), :, cols[t]],
                tail_sems.at[q],
            )
            for q, (i, k, t) in enumerate(tail)
        ]

        head_load.start()
        for s in range(STEPS_BEFORE_HANDSHAKE):
            start_step(s)
        barrier = pltpu.get_barrier_semaphore()
        pl.semaphore_signal(barrier, inc=1, device_id=peer, device_id_type=MESH)
        pl.semaphore_wait(barrier, 1)
        raw_copy.start()
        for s in range(STEPS_BEFORE_HANDSHAKE, last_step):
            start_step(s)
        for load in tail_loads:
            load.start()

        accs = (jnp.zeros((SUBLANES, LANES), jnp.float32),) * tiles
        head_load.wait()
        accs = add_rows(head_buf, accs)
        first = 0
        for b, steps in enumerate(batches):
            wait_all(steps_buf.at[pl.ds(first, steps)], batch_sems.at[b])
            if steps == 1:
                accs = add_step(first, accs)
            else:
                accs = lax.fori_loop(first, first + steps, add_step, accs)
            first += steps

        accs = list(accs)
        for load, (i, k, t) in zip(tail_loads, tail):
            load.wait()
            accs[t] += _tree_sum([steps_buf[last_step, j, :, cols[t]] for j in range(i, i + k)])
            if i + k == STREAMS:
                send_buf[:, cols[t]] = jnp.sum(accs[t], axis=0, keepdims=True)
                pltpu.make_async_remote_copy(
                    send_buf.at[:, cols[t]], recv_buf.at[:, cols[t]], send_sem, recv_sem,
                    device_id=peer, device_id_type=MESH,
                ).start()

        own_load.start()
        own_load.wait()
        accs = add_rows(own_rows, accs)
        raw_copy.wait_recv()
        accs = add_rows(peer_rows, accs)
        o_ref[...] = jnp.concatenate(
            [jnp.sum(a, axis=0, keepdims=True) for a in accs], axis=1
        )
        result = o_ref[...]
        raw_copy.wait_send()
        wait_all(send_buf, send_sem)
        wait_all(recv_buf, recv_sem)
        o_ref[...] = result + recv_buf[...]

    return pl.pallas_call(
        body,
        out_shape=jax.ShapeDtypeStruct((1, n), jnp.float32),
        in_specs=[pl.BlockSpec(memory_space=pl.ANY)],
        out_specs=pl.BlockSpec(memory_space=pltpu.VMEM),
        scratch_shapes=[
            pltpu.VMEM((last_step + 1, STREAMS, SUBLANES, n), jnp.float32),
            pltpu.VMEM((head_rows, n), jnp.float32),
            pltpu.VMEM((RAW_ROWS, n), jnp.float32),
            pltpu.VMEM((RAW_ROWS, n), jnp.float32),
            pltpu.VMEM((1, n), jnp.float32),
            pltpu.VMEM((1, n), jnp.float32),
            pltpu.SemaphoreType.DMA((len(batches),)),
            pltpu.SemaphoreType.DMA((len(tail),)),
            *[pltpu.SemaphoreType.DMA] * 6,
        ],
        compiler_params=pltpu.CompilerParams(
            collective_id=0,
            disable_bounds_checks=True,
            disable_semaphore_checks=True,
        ),
    )(x.reshape(STREAMS + 1, block_rows, n))
```

```python
import jax
import jax.numpy as jnp
from jax import lax
from jax.experimental import pallas as pl
from jax.experimental.pallas import tpu as pltpu

SUBLANES, LANES = 8, 128
MESH = pl.DeviceIdType.MESH

STREAMS = 7
RAW_SLABS = 15
LAST_BATCH_STEPS = (4, 1)
STEPS_BEFORE_HANDSHAKE = 10
UNROLL_SLABS = 8


def _tree_sum(values):
    while len(values) > 1:
        pairs = [values[i] + values[i + 1] for i in range(0, len(values) - 1, 2)]
        values = pairs + values[2 * len(pairs):]
    return values[0]


def pallas_dist_sum_ax0_xy_m2048_n1024_kernel(
    x: jax.Array,
):
    m, n = x.shape
    tiles = n // LANES
    steps = m // SUBLANES // (STREAMS + 1)
    last_step = steps - 1
    head_slabs = steps - RAW_SLABS
    slab_of_step = [head_slabs + s * STREAMS for s in range(steps)]
    batch_ends = [
        slab_of_step[last_step - sum(LAST_BATCH_STEPS[b:])]
        for b in range(len(LAST_BATCH_STEPS) + 1)
    ]
    tail = [(0, STREAMS, t) for t in range(tiles - 1)]
    tail += [(0, STREAMS - 1, tiles - 1), (STREAMS - 1, 1, tiles - 1)]

    def body(x_ref, o_ref, slabs, peer_slabs, own_slabs, send_buf, recv_buf,
             batch_sems, tail_sems, own_sem, raw_send_sem, raw_recv_sem, send_sem, recv_sem):
        peer = (1 - lax.axis_index("x"), lax.axis_index("y"))
        cols = [pl.ds(t * LANES, LANES) for t in range(tiles)]

        def start_step(s):
            batch = sum(slab_of_step[s] >= end for end in batch_ends)
            pltpu.make_async_copy(
                x_ref.at[pl.ds(0, STREAMS), s],
                slabs.at[pl.ds(slab_of_step[s], STREAMS)],
                batch_sems.at[batch],
            ).start()

        def wait_all(buf, sem):
            pltpu.make_async_copy(buf, buf, sem).wait()

        def add_slabs(buf, first, count, accs):
            def add(start, k, accs):
                for i in range(k):
                    accs = tuple(a + buf[start + i, :, c] for a, c in zip(accs, cols))
                return accs

            trips = count // UNROLL_SLABS
            if trips < 2:
                return add(first, count, accs)
            accs = lax.fori_loop(
                0, trips, lambda i, a: add(first + i * UNROLL_SLABS, UNROLL_SLABS, a), accs
            )
            return add(first + trips * UNROLL_SLABS, count % UNROLL_SLABS, accs)

        raw_slabs = x_ref.at[STREAMS, pl.ds(head_slabs, RAW_SLABS)]
        own_load = pltpu.make_async_copy(raw_slabs, own_slabs, own_sem)
        raw_copy = pltpu.make_async_remote_copy(
            raw_slabs, peer_slabs, raw_send_sem, raw_recv_sem,
            device_id=peer, device_id_type=MESH,
        )
        tail_loads = [
            pltpu.make_async_copy(
                x_ref.at[pl.ds(i, k), last_step, :, cols[t]],
                slabs.at[pl.ds(slab_of_step[last_step] + i, k), :, cols[t]],
                tail_sems.at[q],
            )
            for q, (i, k, t) in enumerate(tail)
        ]

        pltpu.make_async_copy(
            x_ref.at[STREAMS, pl.ds(0, head_slabs)],
            slabs.at[pl.ds(0, head_slabs)],
            batch_sems.at[0],
        ).start()
        for s in range(STEPS_BEFORE_HANDSHAKE):
            start_step(s)
        barrier = pltpu.get_barrier_semaphore()
        pl.semaphore_signal(barrier, inc=1, device_id=peer, device_id_type=MESH)
        pl.semaphore_wait(barrier, 1)
        raw_copy.start()
        for s in range(STEPS_BEFORE_HANDSHAKE, last_step):
            start_step(s)
        for load in tail_loads:
            load.start()

        accs = (jnp.zeros((SUBLANES, LANES), jnp.float32),) * tiles
        for b, (first, end) in enumerate(zip([0] + batch_ends, batch_ends)):
            wait_all(slabs.at[pl.ds(first, end - first)], batch_sems.at[b])
            accs = add_slabs(slabs, first, end - first, accs)

        accs = list(accs)
        for load, (i, k, t) in zip(tail_loads, tail):
            load.wait()
            accs[t] += _tree_sum(
                [slabs[slab_of_step[last_step] + j, :, cols[t]] for j in range(i, i + k)]
            )
            if i + k == STREAMS:
                send_buf[:, cols[t]] = jnp.sum(accs[t], axis=0, keepdims=True)
                pltpu.make_async_remote_copy(
                    send_buf.at[:, cols[t]], recv_buf.at[:, cols[t]], send_sem, recv_sem,
                    device_id=peer, device_id_type=MESH,
                ).start()

        own_load.start()
        own_load.wait()
        accs = add_slabs(own_slabs, 0, RAW_SLABS, tuple(accs))
        raw_copy.wait_recv()
        accs = add_slabs(peer_slabs, 0, RAW_SLABS, accs)
        o_ref[...] = jnp.concatenate(
            [jnp.sum(a, axis=0, keepdims=True) for a in accs], axis=1
        )
        result = o_ref[...]
        raw_copy.wait_send()
        wait_all(send_buf, send_sem)
        wait_all(recv_buf, recv_sem)
        o_ref[...] = result + recv_buf[...]

    return pl.pallas_call(
        body,
        out_shape=jax.ShapeDtypeStruct((1, n), jnp.float32),
        in_specs=[pl.BlockSpec(memory_space=pl.ANY)],
        out_specs=pl.BlockSpec(memory_space=pltpu.VMEM),
        scratch_shapes=[
            pltpu.VMEM((m // SUBLANES - RAW_SLABS, SUBLANES, n), jnp.float32),
            pltpu.VMEM((RAW_SLABS, SUBLANES, n), jnp.float32),
            pltpu.VMEM((RAW_SLABS, SUBLANES, n), jnp.float32),
            pltpu.VMEM((1, n), jnp.float32),
            pltpu.VMEM((1, n), jnp.float32),
            pltpu.SemaphoreType.DMA((len(batch_ends),)),
            pltpu.SemaphoreType.DMA((len(tail),)),
            *[pltpu.SemaphoreType.DMA] * 5,
        ],
        compiler_params=pltpu.CompilerParams(
            collective_id=0,
            disable_bounds_checks=True,
            disable_semaphore_checks=True,
        ),
    )(x.reshape(STREAMS + 1, steps, SUBLANES, n))
```

```python
import jax
import jax.numpy as jnp
from jax import lax
from jax.experimental import pallas as pl
from jax.experimental.pallas import tpu as pltpu

SUBLANES, LANES = 8, 128
MESH = pl.DeviceIdType.MESH

STREAMS = 7
RAW_SLABS = 15
LAST_BATCH_STEPS = (4, 1)
STEPS_BEFORE_HANDSHAKE = 10
UNROLL_SLABS = 8


def _tree_sum(values):
    while len(values) > 1:
        pairs = [values[i] + values[i + 1] for i in range(0, len(values) - 1, 2)]
        values = pairs + values[2 * len(pairs):]
    return values[0]


def pallas_dist_sum_ax0_xy_m2048_n1024_kernel(
    x: jax.Array,
):
    m, n = x.shape
    tiles = n // LANES
    steps = m // SUBLANES // (STREAMS + 1)
    last_step = steps - 1
    head_slabs = steps - RAW_SLABS
    slab_of_step = [head_slabs + s * STREAMS for s in range(steps)]
    batch_ends = [
        slab_of_step[last_step - sum(LAST_BATCH_STEPS[b:])]
        for b in range(len(LAST_BATCH_STEPS) + 1)
    ]
    tail = [(0, STREAMS, t) for t in range(tiles - 1)]
    tail += [(0, STREAMS - 1, tiles - 1), (STREAMS - 1, 1, tiles - 1)]

    def body(x_ref, o_ref, slabs, peer_slabs, own_slabs, send_buf, recv_buf,
             batch_sems, tail_sems, own_sem, raw_send_sem, raw_recv_sem, send_sem, recv_sem):
        peer = (1 - lax.axis_index("x"), lax.axis_index("y"))
        cols = [pl.ds(t * LANES, LANES) for t in range(tiles)]

        def start_step(s):
            batch = sum(slab_of_step[s] >= end for end in batch_ends)
            pltpu.make_async_copy(
                x_ref.at[pl.ds(0, STREAMS), s],
                slabs.at[pl.ds(slab_of_step[s], STREAMS)],
                batch_sems.at[batch],
            ).start()

        def wait_all(buf, sem):
            pltpu.make_async_copy(buf, buf, sem).wait()

        def add_slabs(buf, first, count, accs):
            def add(start, k, accs):
                for i in range(k):
                    accs = tuple(a + buf[start + i, :, c] for a, c in zip(accs, cols))
                return accs

            trips = count // UNROLL_SLABS
            if trips < 2:
                return add(first, count, accs)
            accs = lax.fori_loop(
                0, trips, lambda i, a: add(first + i * UNROLL_SLABS, UNROLL_SLABS, a), accs
            )
            return add(first + trips * UNROLL_SLABS, count % UNROLL_SLABS, accs)

        raw_slabs = x_ref.at[STREAMS, pl.ds(head_slabs, RAW_SLABS)]
        own_load = pltpu.make_async_copy(raw_slabs, own_slabs, own_sem)
        raw_copy = pltpu.make_async_remote_copy(
            raw_slabs, peer_slabs, raw_send_sem, raw_recv_sem,
            device_id=peer, device_id_type=MESH,
        )
        tail_loads = [
            pltpu.make_async_copy(
                x_ref.at[pl.ds(i, k), last_step, :, cols[t]],
                slabs.at[pl.ds(slab_of_step[last_step] + i, k), :, cols[t]],
                tail_sems.at[q],
            )
            for q, (i, k, t) in enumerate(tail)
        ]

        pltpu.make_async_copy(
            x_ref.at[STREAMS, pl.ds(0, head_slabs)],
            slabs.at[pl.ds(0, head_slabs)],
            batch_sems.at[0],
        ).start()
        for s in range(STEPS_BEFORE_HANDSHAKE):
            start_step(s)
        barrier = pltpu.get_barrier_semaphore()
        pl.semaphore_signal(barrier, inc=1, device_id=peer, device_id_type=MESH)
        pl.semaphore_wait(barrier, 1)
        raw_copy.start()
        for s in range(STEPS_BEFORE_HANDSHAKE, last_step):
            start_step(s)
        for load in tail_loads:
            load.start()

        zeros = (jnp.zeros((SUBLANES, LANES), jnp.float32),) * tiles
        accs = zeros
        for b, (first, end) in enumerate(zip([0] + batch_ends, batch_ends)):
            wait_all(slabs.at[pl.ds(first, end - first)], batch_sems.at[b])
            accs = add_slabs(slabs, first, end - first, accs)

        accs = list(accs)
        for load, (i, k, t) in zip(tail_loads, tail):
            load.wait()
            accs[t] += _tree_sum(
                [slabs[slab_of_step[last_step] + j, :, cols[t]] for j in range(i, i + k)]
            )
            if i + k == STREAMS:
                send_buf[:, cols[t]] = jnp.sum(accs[t], axis=0, keepdims=True)
                pltpu.make_async_remote_copy(
                    send_buf.at[:, cols[t]], recv_buf.at[:, cols[t]], send_sem, recv_sem,
                    device_id=peer, device_id_type=MESH,
                ).start()

        own_load.start()
        own_load.wait()
        own = add_slabs(own_slabs, 0, RAW_SLABS, zeros)
        raw_copy.wait_recv()
        other = add_slabs(peer_slabs, 0, RAW_SLABS, zeros)
        o_ref[...] = jnp.concatenate(
            [jnp.sum(a + b, axis=0, keepdims=True) for a, b in zip(own, other)], axis=1
        )
        raw_copy.wait_send()
        wait_all(send_buf, send_sem)
        raw_sum, sent = o_ref[...], send_buf[...]
        wait_all(recv_buf, recv_sem)
        o_ref[...] = (sent + recv_buf[...]) + raw_sum

    return pl.pallas_call(
        body,
        out_shape=jax.ShapeDtypeStruct((1, n), jnp.float32),
        in_specs=[pl.BlockSpec(memory_space=pl.ANY)],
        out_specs=pl.BlockSpec(memory_space=pltpu.VMEM),
        scratch_shapes=[
            pltpu.VMEM((m // SUBLANES - RAW_SLABS, SUBLANES, n), jnp.float32),
            pltpu.VMEM((RAW_SLABS, SUBLANES, n), jnp.float32),
            pltpu.VMEM((RAW_SLABS, SUBLANES, n), jnp.float32),
            pltpu.VMEM((1, n), jnp.float32),
            pltpu.VMEM((1, n), jnp.float32),
            pltpu.SemaphoreType.DMA((len(batch_ends),)),
            pltpu.SemaphoreType.DMA((len(tail),)),
            *[pltpu.SemaphoreType.DMA] * 5,
        ],
        compiler_params=pltpu.CompilerParams(
            collective_id=0,
            disable_bounds_checks=True,
            disable_semaphore_checks=True,
        ),
    )(x.reshape(STREAMS + 1, steps, SUBLANES, n))
```
